```python
import numpy as np

kernel_name = "dist_moe_shared_ep_outshard_n512_d256_e2_h512"

def setup_inputs():
    x = np.random.randn(512, 256).astype(np.float32)
    router_W = np.random.randn(256, 8).astype(np.float32) * 0.1
    scores64 = x.astype(np.float64) @ router_W.astype(np.float64)
    route_idx = np.argsort(-scores64, axis=-1)[:, :1].astype(np.int32)
    expert_W = np.random.randn(8, 256, 512).astype(np.float32) * 0.02
    shared_W = np.random.randn(256, 512).astype(np.float32) * 0.02
    return {"x": x, "router_W": router_W, "route_idx": route_idx, "expert_W": expert_W, "shared_W": shared_W}

def reference(x, router_W, route_idx, expert_W, shared_W):
    scores = x @ router_W
    s_max = scores.max(axis=-1, keepdims=True)
    probs = np.exp(scores - s_max)
    probs = probs / probs.sum(axis=-1, keepdims=True)
    shared = x @ shared_W
    out = np.zeros((512, 512), dtype=np.float32)
    for i in range(512):
        e = int(route_idx[i, 0])
        out[i] = shared[i] + probs[i, e] * (x[i] @ expert_W[e])
    return out
```

```python
import jax, jax.numpy as jnp
from jax import lax
from jax.experimental import pallas as pl
from jax.experimental.pallas import tpu as pltpu

N, D, H, E, EL, ND, B = 512, 256, 512, 8, 2, 4, 128
CAP = 32
CLS = (2, 3, 4, 8, 16)
MESH = pl.DeviceIdType.MESH
bf16, f32, i32, u32 = jnp.bfloat16, jnp.float32, jnp.int32, jnp.uint32


def size_switch(n, fn):
    prev = None
    for i, g in enumerate(CLS):
        if prev is None:
            cond = n <= g
        elif i == len(CLS) - 1:
            cond = n > prev
        else:
            cond = jnp.logical_and(n > prev, n <= g)
        pl.when(cond)(lambda g=g: fn(g))
        prev = g


def pallas_dist_moe_shared_ep_outshard_n512_d256_e2_h512_kernel(x, router_W, route_idx, expert_W, shared_W):
    def body(x_hbm, rw_hbm, idx_hbm, ew_hbm, sw_hbm, out_ref,
             xbuf, wbuf, swbuf, rwbuf, idxbuf, sbuf, rbuf, lsem, ssem, rsem):
        my = lax.axis_index("i")
        dk = [(my + k) & 3 for k in range(ND)]
        REM = (2, 1, 3)

        def xcopy(k):
            return pltpu.make_async_copy(x_hbm.at[pl.ds(dk[k] * B, B)], xbuf.at[k], lsem.at[k])
        cidx = [pltpu.make_async_copy(idx_hbm, idxbuf.at[pl.ds(4 * j, 4)], lsem.at[4 + j]) for j in range(2)]
        cw = [pltpu.make_async_copy(ew_hbm.at[e], wbuf.at[e], lsem.at[6 + e]) for e in range(EL)]
        csw = pltpu.make_async_copy(sw_hbm, swbuf, lsem.at[8])
        crw = pltpu.make_async_copy(rw_hbm, rwbuf, lsem.at[9])
        cx = {k: xcopy(k) for k in range(ND)}
        for c in cidx: c.start()
        for k in REM: cx[k].start()
        cw[0].start(); cw[1].start()
        cx[0].start(); crw.start(); csw.start()

        bs = pltpu.get_barrier_semaphore()
        for k in (1, 2, 3):
            pl.semaphore_signal(bs, inc=1, device_id=(dk[k],), device_id_type=MESH)

        r128 = lax.broadcasted_iota(i32, (B, B), 0)
        c128 = lax.broadcasted_iota(i32, (B, B), 1)
        tri = jnp.concatenate([jnp.where(r128 < c128, 1.0, 0.0), jnp.ones((B, B), f32)], axis=1).astype(bf16)
        sub8 = lax.broadcasted_iota(i32, (8, B), 0)
        capio = lax.broadcasted_iota(i32, (CAP, B), 0)
        rowio = lax.broadcasted_iota(i32, (CAP, H // 2), 0)

        for c in cidx: c.wait()
        idx8 = pltpu.roll(idxbuf[...], (8 - my) & 7, 0)
        o_s = idx8 == (2 * my + (sub8 >> 2))
        own = jnp.broadcast_to(idx8[0:1, :], (8, B))
        o_r = own == sub8
        O = jnp.concatenate([jnp.where(o_s, 1.0, 0.0), jnp.where(o_r, 1.0, 0.0)], axis=0).astype(bf16)
        pm = jnp.dot(O, tri, preferred_element_type=f32).astype(i32)
        pos, cnt = pm[:, :B], pm[:, B:]
        v = jnp.where(o_s, pos[0:8], -1)
        ng = jnp.maximum((cnt + 7) >> 3, 1) - 1
        sh4 = sub8 * 4
        pk_s = jnp.sum(ng[0:8] << sh4, axis=0, keepdims=True)
        pk_r = jnp.sum(ng[8:16] << sh4, axis=0, keepdims=True)
        sc_s = pk_s[0, 0]
        sc_r = pk_r[0, 0]

        def n_send(e, k):
            return (lax.shift_right_logical(sc_s, 4 * (4 * e + k)) & 15) + 1

        def n_recv(e, k):
            g = (2 * (my - k) + e) & 7
            return (lax.shift_right_logical(sc_r, 4 * g) & 15) + 1

        def gmat(e, k, r):
            row = jnp.broadcast_to(v[4 * e + k:4 * e + k + 1, :], (CAP, B))
            return jnp.where(row == capio + CAP * r, 1.0, 0.0)

        def expert(e, xg):
            y = jnp.dot(xg, wbuf[e].astype(bf16), preferred_element_type=f32)
            return pltpu.pack_elementwise([y[:, :H // 2], y[:, H // 2:]], packed_dtype=bf16)

        xg = {}
        for k in REM:
            cx[k].wait()
            g2 = jnp.concatenate([gmat(0, k, 0), gmat(1, k, 0)], axis=0).astype(bf16)
            t = jnp.dot(g2, xbuf[k].astype(bf16), preferred_element_type=f32).astype(bf16)
            xg[0, k], xg[1, k] = t[:CAP], t[CAP:]

        def extra_rounds(e, ks, dst):
            nmax = n_send(e, ks[0])
            for k in ks[1:]:
                nmax = jnp.maximum(nmax, n_send(e, k))
            rounds = (nmax + 3) >> 2

            @pl.loop(1, rounds)
            def _(r):
                for k in ks:
                    g = gmat(e, k, r).astype(bf16)
                    t = jnp.dot(g, xbuf[k].astype(bf16), preferred_element_type=f32).astype(bf16)
                    dst(k)[pl.ds(pl.multiple_of(r * CAP, CAP), CAP), :] = expert(e, t)

        def send(e, k, g):
            return pltpu.make_async_remote_copy(
                src_ref=sbuf.at[e, k - 1, pl.ds(0, 8 * g)], dst_ref=rbuf.at[k, e, pl.ds(0, 8 * g)],
                send_sem=ssem.at[3 * e + k - 1], recv_sem=rsem.at[3 * e + k - 1],
                device_id=(dk[k],), device_id_type=MESH)

        for e in range(EL):
            cw[e].wait()
            pk = expert(e, jnp.concatenate([xg[e, k] for k in REM], axis=0))
            for j, k in enumerate(REM):
                sbuf[e, k - 1, 0:CAP, :] = pk[j * CAP:(j + 1) * CAP]
            extra_rounds(e, REM, lambda k: sbuf.at[e, k - 1])
            if e == 0:
                pl.semaphore_wait(bs, 3)
            for k in REM:
                size_switch(n_send(e, k), lambda g: send(e, k, g).start())

        cx[0].wait()
        xo = xbuf[0]
        xob = xo.astype(bf16)
        g2 = jnp.concatenate([gmat(0, 0, 0), gmat(1, 0, 0)], axis=0).astype(bf16)
        t = jnp.dot(g2, xob, preferred_element_type=f32).astype(bf16)
        for e in range(EL):
            rbuf[0, e, 0:CAP, :] = expert(e, t[e * CAP:(e + 1) * CAP])
            extra_rounds(e, (0,), lambda k: rbuf.at[0, e])

        crw.wait()
        sc = lax.dot_general(rwbuf[...], xo, (((1,), (1,)), ((), ())), preferred_element_type=f32,
                             precision=lax.Precision.HIGHEST)
        ex = jnp.exp(sc - jnp.max(sc, axis=0, keepdims=True))
        p_row = jnp.sum(jnp.where(o_r, ex, 0.0), axis=0, keepdims=True) / jnp.sum(ex, axis=0, keepdims=True)
        pcol = jnp.broadcast_to(p_row, (B, B)).T
        rank = jnp.sum(jnp.where(o_r, pos[8:16], 0), axis=0, keepdims=True)
        gi = idx8[0:1, :]
        base = 128 * ((my - (gi >> 1)) & 3) + 64 * (gi & 1)
        okg = jnp.logical_and(gi >= 0, gi < E)

        def code_t(r):
            rr = rank - CAP * r
            ok = jnp.logical_and(okg, jnp.logical_and(rr >= 0, rr < CAP))
            code = jnp.where(ok, base + 2 * rr, -1024)
            return jnp.broadcast_to(code, (B, B)).T

        def smat(ct, k, h):
            return jnp.where(ct - (128 * k - h) == c128, 1.0, 0.0).astype(bf16)

        def bmat(k, r):
            parts = []
            for e in range(EL):
                rows = rbuf[k, e, pl.ds(r * CAP, CAP), :]
                parts.append(jnp.where(rowio + r * CAP < 8 * n_recv(e, k), rows, jnp.uint32(0)))
            return pltpu.bitcast(jnp.concatenate(parts, axis=0), bf16)

        def accumulate(k, r, ct):
            bm = bmat(k, r)
            for h in range(2):
                y = jnp.dot(smat(ct, k, h), bm, preferred_element_type=f32)
                for c in range(2):
                    cols = slice(256 * h + 128 * c, 256 * h + 128 * (c + 1))
                    out_ref[:, cols] += pcol * y[:, 128 * c:128 * (c + 1)]

        ct0 = code_t(0)
        csw.wait()
        out_ref[...] = jnp.dot(xob, swbuf[...].astype(bf16), preferred_element_type=f32)
        accumulate(0, 0, ct0)
        for k in (1, 3, 2):
            for e in range(EL):
                size_switch(n_recv(e, k), lambda g: send(e, k, g).wait_recv())
            if k == 3:
                for e in range(EL):
                    for kk in REM:
                        size_switch(n_send(e, kk), lambda g: send(e, kk, g).wait_send())
            accumulate(k, 0, ct0)

        nmax = n_recv(0, 0)
        for e in range(EL):
            for k in range(ND):
                nmax = jnp.maximum(nmax, n_recv(e, k))

        @pl.loop(1, (nmax + 3) >> 2)
        def _(r):
            ct = code_t(r)
            for k in range(ND):
                accumulate(k, pl.multiple_of(r, 1), ct)

    ANY = pl.BlockSpec(memory_space=pl.ANY)
    return pl.pallas_call(
        body,
        out_shape=jax.ShapeDtypeStruct((B, H), f32),
        in_specs=[ANY] * 5,
        out_specs=pl.BlockSpec(memory_space=pltpu.VMEM),
        scratch_shapes=[
            pltpu.VMEM((ND, B, D), f32), pltpu.VMEM((EL, D, H), f32), pltpu.VMEM((D, H), f32),
            pltpu.VMEM((E, D), f32), pltpu.VMEM((8, B), i32),
            pltpu.VMEM((EL, 3, B, H // 2), u32), pltpu.VMEM((ND, EL, B, H // 2), u32),
            pltpu.SemaphoreType.DMA((10,)), pltpu.SemaphoreType.DMA((6,)), pltpu.SemaphoreType.DMA((6,)),
        ],
        compiler_params=pltpu.CompilerParams(collective_id=0, disable_semaphore_checks=True, disable_bounds_checks=True),
    )(x, router_W.T, route_idx.reshape(4, B), expert_W, shared_W)
```

```python
import jax
import jax.numpy as jnp
from jax import lax
from jax.experimental import pallas as pl
from jax.experimental.pallas import tpu as pltpu

D, H, E, EL, ND, B = 256, 512, 8, 2, 4, 128
CAP = 32
GR = 4
CLS = (16, 20, 24, 32)
REM = (2, 1, 3)
PHASES = ((0, 0), (1, 0), (0, 1), (1, 1))
SENDS = (
    ((0, 2), (0, 1), (0, 3)),
    ((1, 2), (1, 1), (1, 3)),
    ((2, 2),),
    ((3, 2), (2, 1), (2, 3), (3, 1), (3, 3)),
)
MESH = pl.DeviceIdType.MESH
bf16, f32, i32, u32 = jnp.bfloat16, jnp.float32, jnp.int32, jnp.uint32


def _size_switch(n, fn):
    prev = None
    for i, g in enumerate(CLS):
        if prev is None:
            cond = n <= g
        elif i == len(CLS) - 1:
            cond = n > prev
        elif g - prev == GR:
            cond = n == g
        else:
            cond = jnp.logical_and(n > prev, n <= g)
        pl.when(cond)(lambda g=g: fn(g))
        prev = g


def _body(x_hbm, rw_hbm, idx_hbm, ew_hbm, sw_hbm, out_ref,
          xbuf, wbuf, swbuf, rwbuf, idxbuf, sbuf, rbuf, lsem, wsem, ssem, rsem):
    my = lax.axis_index("i")
    dk = [(my + k) & 3 for k in range(ND)]

    cx = [pltpu.make_async_copy(x_hbm.at[pl.ds(dk[k] * B, B)], xbuf.at[k], lsem.at[k])
          for k in range(ND)]
    cidx = [pltpu.make_async_copy(idx_hbm, idxbuf.at[pl.ds(4 * j, 4)], lsem.at[4 + j])
            for j in range(2)]
    cw = {(e, h): pltpu.make_async_copy(ew_hbm.at[e, :, pl.ds(256 * h, 256)],
                                        wbuf.at[e, :, pl.ds(256 * h, 256)],
                                        wsem.at[2 * e + h])
          for e in range(EL) for h in range(2)}
    csw = pltpu.make_async_copy(sw_hbm, swbuf, lsem.at[6])
    crw = pltpu.make_async_copy(rw_hbm, rwbuf, lsem.at[7])
    for c in cidx:
        c.start()
    for k in REM:
        cx[k].start()
    barrier = pltpu.get_barrier_semaphore()
    for k in (1, 2, 3):
        pl.semaphore_signal(barrier, inc=1, device_id=(dk[k],), device_id_type=MESH)
    for ph in PHASES:
        cw[ph].start()

    r128 = lax.broadcasted_iota(i32, (B, B), 0)
    c128 = lax.broadcasted_iota(i32, (B, B), 1)
    tri = jnp.concatenate([jnp.where(r128 < c128, 1.0, 0.0), jnp.ones((B, B), f32)],
                          axis=1).astype(bf16)
    sub8 = lax.broadcasted_iota(i32, (8, B), 0)
    capio = lax.broadcasted_iota(i32, (CAP, B), 0)

    for c in cidx:
        c.wait()
    idx8 = pltpu.roll(idxbuf[...], (8 - my) & 7, 0)
    mine = idx8 == (2 * my + (sub8 >> 2))
    hot = [jnp.broadcast_to(idx8[k:k + 1, :], (8, B)) == sub8 for k in range(ND)]
    onehots = jnp.concatenate([jnp.where(m, 1.0, 0.0) for m in [mine] + hot]
                              + [jnp.zeros((8, B), f32)], axis=0).astype(bf16)
    pm = jnp.dot(onehots, tri, preferred_element_type=f32)
    pos = pm[0:16, :B].astype(i32)
    cnt = pm[0:16, B:].astype(i32)
    slot = jnp.where(mine, pos[0:8], -1)
    groups = jnp.minimum(jnp.maximum((cnt + GR - 1) >> 2, 1) - 1, 15)
    nib = sub8 * 4
    send_word = jnp.sum(groups[0:8] << nib, axis=0, keepdims=True)[0, 0]
    recv_word = jnp.sum(groups[8:16] << nib, axis=0, keepdims=True)[0, 0]
    cmax = jnp.maximum(jnp.maximum(pm[8:16, B:], pm[16:24, B:]),
                       jnp.maximum(pm[24:32, B:], pm[32:40, B:]))
    generic = jnp.max(cmax, axis=0, keepdims=True)[0, 0] > float(CAP)

    n_send = {(e, k): GR * ((lax.shift_right_logical(send_word, 4 * (4 * e + k)) & 15) + 1)
              for e in range(EL) for k in REM}
    n_recv = {(e, k): GR * ((lax.shift_right_logical(recv_word, 4 * ((2 * (my - k) + e) & 7)) & 15) + 1)
              for e in range(EL) for k in REM}

    rank = jnp.sum(jnp.where(hot[0], pos[8:16], 0), axis=0, keepdims=True)
    route = idx8[0:1, :]
    k_of = (my - (route >> 1)) & 3
    in_range = jnp.logical_and(route >= 0, route < E)

    def gather_mat(e, k, r):
        row = jnp.broadcast_to(slot[4 * e + k:4 * e + k + 1, :], (CAP, B))
        return jnp.where(row == capio + CAP * r, 1.0, 0.0)

    def w_piece(e, h):
        return wbuf[e, :, 256 * h:256 * h + 256].astype(bf16)

    def expert(e, h, xg):
        y = jnp.dot(xg, w_piece(e, h), preferred_element_type=f32)
        return pltpu.pack_elementwise([y[:, :B], y[:, B:]], packed_dtype=bf16)

    def flow(e, h, k, rows):
        j = (2 * e + h) * 3 + k - 1
        return pltpu.make_async_remote_copy(
            src_ref=sbuf.at[e, h, k - 1, pl.ds(0, rows)],
            dst_ref=rbuf.at[k, h, e, pl.ds(0, rows)],
            send_sem=ssem.at[j], recv_sem=rsem.at[j],
            device_id=(dk[k],), device_id_type=MESH)

    def prob_col(xo):
        sc = lax.dot_general(rwbuf[...].astype(bf16), xo.astype(bf16), (((1,), (1,)), ((), ())),
                             preferred_element_type=f32)
        ex = jnp.exp(sc - jnp.max(sc, axis=0, keepdims=True))
        p = jnp.sum(jnp.where(hot[0], ex, 0.0), axis=0, keepdims=True) / jnp.sum(ex, axis=0, keepdims=True)
        return jnp.broadcast_to(p, (B, B)).T

    def slot_col(r, place):
        rr = rank - CAP * r
        ok = jnp.logical_and(in_range, jnp.logical_and(rr >= 0, rr < CAP))
        code = jnp.where(ok, 64 * place + 32 * (route & 1) + rr, -1024)
        return jnp.broadcast_to(code, (B, B)).T

    def scatter_mat(col, off):
        return jnp.where(col - off == c128, 1.0, 0.0).astype(bf16)

    def received(k, h, r, masked):
        los, his = [], []
        for e in range(EL):
            rows = rbuf[k, h, e, pl.ds(r * CAP, CAP), :]
            if masked:
                rows = jnp.where(capio < n_recv[e, k], rows, jnp.uint32(0))
            los.append(pltpu.unpack_elementwise(rows, index=0, packed_dtype=bf16, unpacked_dtype=f32))
            his.append(pltpu.unpack_elementwise(rows, index=1, packed_dtype=bf16, unpacked_dtype=f32))
        lo = jnp.concatenate(los, axis=0).astype(bf16)
        hi = jnp.concatenate(his, axis=0).astype(bf16)
        return jnp.concatenate([lo, hi], axis=1)

    def add_out(h, p, y):
        for t in range(2):
            cols = slice(256 * h + 128 * t, 256 * h + 128 * (t + 1))
            out_ref[:, cols] += p * y[:, 128 * t:128 * (t + 1)]

    @pl.when(jnp.logical_not(generic))
    def _fast():
        xg = {}
        for k in REM:
            cx[k].wait()
            g = jnp.concatenate([gather_mat(0, k, 0), gather_mat(1, k, 0)], axis=0).astype(bf16)
            t = jnp.dot(g, xbuf[k].astype(bf16), preferred_element_type=f32).astype(bf16)
            xg[0, k], xg[1, k] = t[:CAP], t[CAP:]
        xg = [jnp.concatenate([xg[e, k] for k in REM], axis=0) for e in range(EL)]

        col = slot_col(0, jnp.where(k_of == 1, 0, jnp.where(k_of == 3, 1, jnp.where(k_of == 2, 2, 3))))
        s_near, s_far = scatter_mat(col, 0), scatter_mat(col, 128)

        def start(items):
            for ph, k in items:
                e, h = PHASES[ph]
                _size_switch(n_send[e, k], lambda rows, e=e, h=h, k=k: flow(e, h, k, rows).start())

        for i, (e, h) in enumerate(PHASES):
            cw[e, h].wait()
            if i == len(PHASES) - 1:
                cx[0].start()
                crw.start()
                csw.start()
            packed = expert(e, h, xg[e])
            sbuf[e, h, 1, 0:CAP, :] = packed[0:CAP]
            if i == 0:
                pl.semaphore_wait(barrier, 3)
            start(SENDS[i][:1])
            sbuf[e, h, 0, 0:CAP, :] = packed[CAP:2 * CAP]
            sbuf[e, h, 2, 0:CAP, :] = packed[2 * CAP:3 * CAP]
            start(SENDS[i][1:])

        cx[0].wait()
        crw.wait()
        xo = xbuf[0]
        p = prob_col(xo)
        x_e = []
        for e in range(EL):
            m = jnp.where((col >> 5) == 6 + e, 1.0, 0.0)
            x_e.append(jnp.concatenate([xo[:, :B] * m, xo[:, B:] * m], axis=1).astype(bf16))
        csw.wait()
        xo16 = xo.astype(bf16)
        for h in range(2):
            y_sh = jnp.dot(xo16, swbuf[:, 256 * h:256 * h + 256].astype(bf16), preferred_element_type=f32)
            y_ex = (jnp.dot(x_e[0], w_piece(0, h), preferred_element_type=f32)
                    + jnp.dot(x_e[1], w_piece(1, h), preferred_element_type=f32))
            for t in range(2):
                cs = slice(128 * t, 128 * (t + 1))
                out_ref[:, 256 * h + 128 * t:256 * h + 128 * (t + 1)] = y_sh[:, cs] + p * y_ex[:, cs]

        for e in range(EL):
            for h in range(2):
                for k in REM:
                    _size_switch(n_send[e, k], lambda rows, e=e, h=h, k=k: flow(e, h, k, rows).wait_send())

        def wait_recv(k, h):
            for e in range(EL):
                _size_switch(n_recv[e, k], lambda rows, e=e: flow(e, h, k, rows).wait_recv())

        for k in (1, 3):
            for h in range(2):
                wait_recv(k, h)
        wait_recv(2, 0)
        zpad = jnp.zeros((64, 256), bf16)
        for h in range(2):
            near = jnp.concatenate([received(1, h, 0, True), received(3, h, 0, True)], axis=0)
            y = jnp.dot(s_near, near, preferred_element_type=f32)
            if h == 0:
                far = jnp.concatenate([received(2, h, 0, True), zpad], axis=0)
                y = y + jnp.dot(s_far, far, preferred_element_type=f32)
            add_out(h, p, y)

        wait_recv(2, 1)
        far = jnp.concatenate([received(2, 1, 0, True), zpad], axis=0)
        for t in range(2):
            for mh in range(2):
                rows = slice(64 * mh, 64 * mh + 64)
                cols = slice(256 + 128 * t, 256 + 128 * (t + 1))
                y = jnp.dot(s_far[rows], far[:, 128 * t:128 * (t + 1)], preferred_element_type=f32)
                out_ref[rows, cols] += p[rows] * y

    @pl.when(generic)
    def _generic():
        cx[0].start()
        crw.start()
        csw.start()
        for k in range(ND):
            cx[k].wait()
        for ph in PHASES:
            cw[ph].wait()
        crw.wait()
        csw.wait()
        pl.semaphore_wait(barrier, 3)

        @pl.loop(0, B // CAP)
        def _(r):
            for k in range(ND):
                for e in range(EL):
                    g = gather_mat(e, k, r).astype(bf16)
                    t = jnp.dot(g, xbuf[k].astype(bf16), preferred_element_type=f32).astype(bf16)
                    for h in range(2):
                        dst = rbuf.at[0, h, e] if k == 0 else sbuf.at[e, h, k - 1]
                        dst[pl.ds(pl.multiple_of(r * CAP, CAP), CAP), :] = expert(e, h, t)

        every = [(e, h, k) for e in range(EL) for h in range(2) for k in REM]
        for e, h, k in every:
            flow(e, h, k, B).start()
        xo = xbuf[0]
        p = prob_col(xo)
        out_ref[...] = jnp.dot(xo.astype(bf16), swbuf[...].astype(bf16), preferred_element_type=f32)
        for e, h, k in every:
            flow(e, h, k, B).wait()

        @pl.loop(0, B // CAP)
        def _(r):
            col = slot_col(r, k_of)
            s01, s23 = scatter_mat(col, 0), scatter_mat(col, 128)
            for h in range(2):
                b01 = jnp.concatenate([received(0, h, r, False), received(1, h, r, False)], axis=0)
                b23 = jnp.concatenate([received(2, h, r, False), received(3, h, r, False)], axis=0)
                y = (jnp.dot(s01, b01, preferred_element_type=f32)
                     + jnp.dot(s23, b23, preferred_element_type=f32))
                add_out(h, p, y)


def pallas_dist_moe_shared_ep_outshard_n512_d256_e2_h512_kernel(
    x: jax.Array,
    router_W: jax.Array,
    route_idx: jax.Array,
    expert_W: jax.Array,
    shared_W: jax.Array,
):
    any_space = pl.BlockSpec(memory_space=pl.ANY)
    return pl.pallas_call(
        _body,
        out_shape=jax.ShapeDtypeStruct((B, H), f32),
        in_specs=[any_space] * 5,
        out_specs=pl.BlockSpec(memory_space=pltpu.VMEM),
        scratch_shapes=[
            pltpu.VMEM((ND, B, D), f32),
            pltpu.VMEM((EL, D, H), f32),
            pltpu.VMEM((D, H), f32),
            pltpu.VMEM((E, D), f32),
            pltpu.VMEM((8, B), i32),
            pltpu.VMEM((EL, 2, 3, B, B), u32),
            pltpu.VMEM((ND, 2, EL, B, B), u32),
            pltpu.SemaphoreType.DMA((8,)),
            pltpu.SemaphoreType.DMA((4,)),
            pltpu.SemaphoreType.DMA((12,)),
            pltpu.SemaphoreType.DMA((12,)),
        ],
        compiler_params=pltpu.CompilerParams(
            collective_id=0,
            disable_semaphore_checks=True,
            disable_bounds_checks=True,
        ),
    )(x, router_W.T, route_idx.reshape(ND, B), expert_W, shared_W)
```

```python
import jax
import jax.numpy as jnp
from jax import lax
from jax.experimental import pallas as pl
from jax.experimental.pallas import tpu as pltpu

D, H, E, EL, ND, B = 256, 512, 8, 2, 4, 128
CAP = 32
GR = 4
CLS = (16, 20, 24, 32)
REM = (2, 3, 1)
PHASES = ((0, 0), (1, 0), (0, 1), (1, 1))
SENDS = (
    ((0, 2), (0, 3)),
    ((1, 2), (1, 3)),
    ((2, 2),),
    ((3, 2), (2, 3), (3, 3)),
)
MESH = pl.DeviceIdType.MESH
bf16, f32, i32, u32 = jnp.bfloat16, jnp.float32, jnp.int32, jnp.uint32


def _size_switch(n, fn):
    prev = None
    for i, g in enumerate(CLS):
        if prev is None:
            cond = n <= g
        elif i == len(CLS) - 1:
            cond = n > prev
        elif g - prev == GR:
            cond = n == g
        else:
            cond = jnp.logical_and(n > prev, n <= g)
        pl.when(cond)(lambda g=g: fn(g))
        prev = g


def _body(x_hbm, rw_hbm, idx_hbm, ew_hbm, sw_hbm, out_ref,
          xbuf, wbuf, swbuf, rwbuf, idxbuf, sbuf, rbuf, lsem, wsem, ssem, rsem):
    my = lax.axis_index("i")
    dk = [(my + k) & 3 for k in range(ND)]

    cx = [pltpu.make_async_copy(x_hbm.at[pl.ds(dk[k] * B, B)], xbuf.at[k], lsem.at[k])
          for k in range(ND)]
    cidx = [pltpu.make_async_copy(idx_hbm, idxbuf.at[pl.ds(4 * j, 4)], lsem.at[4 + j])
            for j in range(2)]
    cw = {(e, h): pltpu.make_async_copy(ew_hbm.at[e, :, pl.ds(256 * h, 256)],
                                        wbuf.at[e, :, pl.ds(256 * h, 256)],
                                        wsem.at[2 * e + h])
          for e in range(EL) for h in range(2)}
    csw = pltpu.make_async_copy(sw_hbm, swbuf, lsem.at[6])
    crw = pltpu.make_async_copy(rw_hbm, rwbuf, lsem.at[7])
    for c in cidx:
        c.start()
    for k in (2, 3):
        cx[k].start()
    barrier = pltpu.get_barrier_semaphore()
    for k in (1, 2, 3):
        pl.semaphore_signal(barrier, inc=1, device_id=(dk[k],), device_id_type=MESH)
    for ph in PHASES:
        cw[ph].start()

    r128 = lax.broadcasted_iota(i32, (B, B), 0)
    c128 = lax.broadcasted_iota(i32, (B, B), 1)
    tri = jnp.concatenate([jnp.where(r128 < c128, 1.0, 0.0), jnp.ones((B, B), f32)],
                          axis=1).astype(bf16)
    sub8 = lax.broadcasted_iota(i32, (8, B), 0)
    capio = lax.broadcasted_iota(i32, (CAP, B), 0)

    for c in cidx:
        c.wait()
    cx[1].start()
    idx8 = pltpu.roll(idxbuf[...], (8 - my) & 7, 0)
    mine = idx8 == (2 * my + (sub8 >> 2))
    hot = [jnp.broadcast_to(idx8[k:k + 1, :], (8, B)) == sub8 for k in range(ND)]
    onehots = jnp.concatenate([jnp.where(m, 1.0, 0.0) for m in [mine] + hot]
                              + [jnp.zeros((8, B), f32)], axis=0).astype(bf16)
    pm = jnp.dot(onehots, tri, preferred_element_type=f32)
    pos = pm[0:16, :B].astype(i32)
    cnt = pm[0:16, B:].astype(i32)
    slot = jnp.where(mine, pos[0:8], -1)
    groups = jnp.minimum(jnp.maximum((cnt + GR - 1) >> 2, 1) - 1, 15)
    nib = sub8 * 4
    send_word = jnp.sum(groups[0:8] << nib, axis=0, keepdims=True)[0, 0]
    recv_word = jnp.sum(groups[8:16] << nib, axis=0, keepdims=True)[0, 0]
    cmax = jnp.maximum(jnp.maximum(pm[8:16, B:], pm[16:24, B:]),
                       jnp.maximum(pm[24:32, B:], pm[32:40, B:]))
    generic = jnp.max(cmax, axis=0, keepdims=True)[0, 0] > float(CAP)

    n_send = {(e, k): GR * ((lax.shift_right_logical(send_word, 4 * (4 * e + k)) & 15) + 1)
              for e in range(EL) for k in REM}
    n_recv = {(e, k): GR * ((lax.shift_right_logical(recv_word, 4 * ((2 * (my - k) + e) & 7)) & 15) + 1)
              for e in range(EL) for k in REM}

    rank = jnp.sum(jnp.where(hot[0], pos[8:16], 0), axis=0, keepdims=True)
    route = idx8[0:1, :]
    k_of = (my - (route >> 1)) & 3
    in_range = jnp.logical_and(route >= 0, route < E)

    def gather_mat(e, k, r):
        row = jnp.broadcast_to(slot[4 * e + k:4 * e + k + 1, :], (CAP, B))
        return jnp.where(row == capio + CAP * r, 1.0, 0.0)

    def w_piece(e, h):
        return wbuf[e, :, 256 * h:256 * h + 256].astype(bf16)

    def expert(e, h, xg):
        y = jnp.dot(xg, w_piece(e, h), preferred_element_type=f32)
        return pltpu.pack_elementwise([y[:, :B], y[:, B:]], packed_dtype=bf16)

    def flow(e, h, k, rows):
        j = (2 * e + h) * 3 + k - 1
        return pltpu.make_async_remote_copy(
            src_ref=sbuf.at[e, h, k - 1, pl.ds(0, rows)],
            dst_ref=rbuf.at[k, h, e, pl.ds(0, rows)],
            send_sem=ssem.at[j], recv_sem=rsem.at[j],
            device_id=(dk[k],), device_id_type=MESH)

    def prob_col(xo):
        sc = lax.dot_general(rwbuf[...].astype(bf16), xo.astype(bf16), (((1,), (1,)), ((), ())),
                             preferred_element_type=f32)
        ex = jnp.exp(sc - jnp.max(sc, axis=0, keepdims=True))
        p = jnp.sum(jnp.where(hot[0], ex, 0.0), axis=0, keepdims=True) / jnp.sum(ex, axis=0, keepdims=True)
        return jnp.broadcast_to(p, (B, B)).T

    def slot_col(r, place):
        rr = rank - CAP * r
        ok = jnp.logical_and(in_range, jnp.logical_and(rr >= 0, rr < CAP))
        code = jnp.where(ok, 64 * place + 32 * (route & 1) + rr, -1024)
        return jnp.broadcast_to(code, (B, B)).T

    def scatter_mat(col, off):
        return jnp.where(col - off == c128, 1.0, 0.0).astype(bf16)

    def received(k, h, r, masked):
        los, his = [], []
        for e in range(EL):
            rows = rbuf[k, h, e, pl.ds(r * CAP, CAP), :]
            if masked:
                rows = jnp.where(capio < n_recv[e, k], rows, jnp.uint32(0))
            los.append(pltpu.unpack_elementwise(rows, index=0, packed_dtype=bf16, unpacked_dtype=f32))
            his.append(pltpu.unpack_elementwise(rows, index=1, packed_dtype=bf16, unpacked_dtype=f32))
        lo = jnp.concatenate(los, axis=0).astype(bf16)
        hi = jnp.concatenate(his, axis=0).astype(bf16)
        return jnp.concatenate([lo, hi], axis=1)

    def add_out(h, p, y):
        for t in range(2):
            cols = slice(256 * h + 128 * t, 256 * h + 128 * (t + 1))
            out_ref[:, cols] += p * y[:, 128 * t:128 * (t + 1)]

    @pl.when(jnp.logical_not(generic))
    def _fast():
        def gather(k):
            cx[k].wait()
            g = jnp.concatenate([gather_mat(0, k, 0), gather_mat(1, k, 0)], axis=0).astype(bf16)
            t = jnp.dot(g, xbuf[k].astype(bf16), preferred_element_type=f32).astype(bf16)
            return t[:CAP], t[CAP:]

        x2, x3 = gather(2), gather(3)
        xg = [jnp.concatenate([x2[e], x3[e]], axis=0) for e in range(EL)]

        col = slot_col(0, jnp.where(k_of == 3, 0, jnp.where(k_of == 2, 1, jnp.where(k_of == 1, 2, 3))))
        s_32, s_1 = scatter_mat(col, 0), scatter_mat(col, 128)

        def start(items):
            for ph, k in items:
                e, h = PHASES[ph]
                _size_switch(n_send[e, k], lambda rows, e=e, h=h, k=k: flow(e, h, k, rows).start())

        for i, (e, h) in enumerate(PHASES):
            cw[e, h].wait()
            if i == len(PHASES) - 1:
                cx[0].start()
                crw.start()
                csw.start()
            packed = expert(e, h, xg[e])
            sbuf[e, h, 1, 0:CAP, :] = packed[0:CAP]
            if i == 0:
                pl.semaphore_wait(barrier, 3)
            start(SENDS[i][:1])
            sbuf[e, h, 2, 0:CAP, :] = packed[CAP:2 * CAP]
            start(SENDS[i][1:])

        x1 = gather(1)
        for e in range(EL):
            y = jnp.dot(x1[e], wbuf[e].astype(bf16), preferred_element_type=f32)
            for h in range(2):
                sbuf[e, h, 0, 0:CAP, :] = pltpu.pack_elementwise(
                    [y[:, 256 * h:256 * h + B], y[:, 256 * h + B:256 * h + 256]], packed_dtype=bf16)
            for h in range(2):
                _size_switch(n_send[e, 1], lambda rows, e=e, h=h: flow(e, h, 1, rows).start())

        cx[0].wait()
        crw.wait()
        xo = xbuf[0]
        p = prob_col(xo)
        x_e = []
        for e in range(EL):
            m = jnp.where((col >> 5) == 6 + e, 1.0, 0.0)
            x_e.append(jnp.concatenate([xo[:, :B] * m, xo[:, B:] * m], axis=1).astype(bf16))
        csw.wait()
        xo16 = xo.astype(bf16)
        for h in range(2):
            y_sh = jnp.dot(xo16, swbuf[:, 256 * h:256 * h + 256].astype(bf16), preferred_element_type=f32)
            y_ex = (jnp.dot(x_e[0], w_piece(0, h), preferred_element_type=f32)
                    + jnp.dot(x_e[1], w_piece(1, h), preferred_element_type=f32))
            for t in range(2):
                cs = slice(128 * t, 128 * (t + 1))
                out_ref[:, 256 * h + 128 * t:256 * h + 128 * (t + 1)] = y_sh[:, cs] + p * y_ex[:, cs]

        for e in range(EL):
            for h in range(2):
                for k in REM:
                    _size_switch(n_send[e, k], lambda rows, e=e, h=h, k=k: flow(e, h, k, rows).wait_send())

        def wait_recv(k, h):
            for e in range(EL):
                _size_switch(n_recv[e, k], lambda rows, e=e: flow(e, h, k, rows).wait_recv())

        zpad = jnp.zeros((64, 256), bf16)
        for h in range(2):
            wait_recv(3, h)
        wait_recv(2, 0)
        for h in range(2):
            second = received(2, 0, 0, True) if h == 0 else zpad
            rows = jnp.concatenate([received(3, h, 0, True), second], axis=0)
            add_out(h, p, jnp.dot(s_32, rows, preferred_element_type=f32))
        for h in range(2):
            wait_recv(1, h)
        for h in range(2):
            rows = jnp.concatenate([received(1, h, 0, True), zpad], axis=0)
            add_out(h, p, jnp.dot(s_1, rows, preferred_element_type=f32))
        wait_recv(2, 1)
        far = jnp.concatenate([zpad, received(2, 1, 0, True)], axis=0)
        for t in range(2):
            for mh in range(2):
                rows = slice(64 * mh, 64 * mh + 64)
                cols = slice(256 + 128 * t, 256 + 128 * (t + 1))
                y = jnp.dot(s_32[rows], far[:, 128 * t:128 * (t + 1)], preferred_element_type=f32)
                out_ref[rows, cols] += p[rows] * y

    @pl.when(generic)
    def _generic():
        cx[0].start()
        crw.start()
        csw.start()
        for k in range(ND):
            cx[k].wait()
        for ph in PHASES:
            cw[ph].wait()
        crw.wait()
        csw.wait()
        pl.semaphore_wait(barrier, 3)

        @pl.loop(0, B // CAP)
        def _(r):
            for k in range(ND):
                for e in range(EL):
                    g = gather_mat(e, k, r).astype(bf16)
                    t = jnp.dot(g, xbuf[k].astype(bf16), preferred_element_type=f32).astype(bf16)
                    for h in range(2):
                        dst = rbuf.at[0, h, e] if k == 0 else sbuf.at[e, h, k - 1]
                        dst[pl.ds(pl.multiple_of(r * CAP, CAP), CAP), :] = expert(e, h, t)

        every = [(e, h, k) for e in range(EL) for h in range(2) for k in REM]
        for e, h, k in every:
            flow(e, h, k, B).start()
        xo = xbuf[0]
        p = prob_col(xo)
        out_ref[...] = jnp.dot(xo.astype(bf16), swbuf[...].astype(bf16), preferred_element_type=f32)
        for e, h, k in every:
            flow(e, h, k, B).wait()

        @pl.loop(0, B // CAP)
        def _(r):
            col = slot_col(r, k_of)
            s01, s23 = scatter_mat(col, 0), scatter_mat(col, 128)
            for h in range(2):
                b01 = jnp.concatenate([received(0, h, r, False), received(1, h, r, False)], axis=0)
                b23 = jnp.concatenate([received(2, h, r, False), received(3, h, r, False)], axis=0)
                y = (jnp.dot(s01, b01, preferred_element_type=f32)
                     + jnp.dot(s23, b23, preferred_element_type=f32))
                add_out(h, p, y)


def pallas_dist_moe_shared_ep_outshard_n512_d256_e2_h512_kernel(
    x: jax.Array,
    router_W: jax.Array,
    route_idx: jax.Array,
    expert_W: jax.Array,
    shared_W: jax.Array,
):
    any_space = pl.BlockSpec(memory_space=pl.ANY)
    return pl.pallas_call(
        _body,
        out_shape=jax.ShapeDtypeStruct((B, H), f32),
        in_specs=[any_space] * 5,
        out_specs=pl.BlockSpec(memory_space=pltpu.VMEM),
        scratch_shapes=[
            pltpu.VMEM((ND, B, D), f32),
            pltpu.VMEM((EL, D, H), f32),
            pltpu.VMEM((D, H), f32),
            pltpu.VMEM((E, D), f32),
            pltpu.VMEM((8, B), i32),
            pltpu.VMEM((EL, 2, 3, B, B), u32),
            pltpu.VMEM((ND, 2, EL, B, B), u32),
            pltpu.SemaphoreType.DMA((8,)),
            pltpu.SemaphoreType.DMA((4,)),
            pltpu.SemaphoreType.DMA((12,)),
            pltpu.SemaphoreType.DMA((12,)),
        ],
        compiler_params=pltpu.CompilerParams(
            collective_id=0,
            disable_semaphore_checks=True,
            disable_bounds_checks=True,
        ),
    )(x, router_W.T, route_idx.reshape(ND, B), expert_W, shared_W)
```

```python
import jax
import jax.numpy as jnp
from jax import lax
from jax.experimental import pallas as pl
from jax.experimental.pallas import tpu as pltpu

D, H, E, EL, ND, B = 256, 512, 8, 2, 4, 128
CAP = 32
GR = 4
CLS = (16, 20, 24, 32)
REM = (2, 3, 1)
PHASES = ((0, 0), (1, 0), (0, 1), (1, 1))
SENDS = (
    ((0, 2), (0, 3)),
    ((1, 2), (1, 3)),
    ((2, 2),),
    ((3, 2), (2, 3), (3, 3)),
)
MESH = pl.DeviceIdType.MESH
bf16, f32, i32, u32 = jnp.bfloat16, jnp.float32, jnp.int32, jnp.uint32


def _size_switch(n, fn):
    prev = None
    for i, g in enumerate(CLS):
        if prev is None:
            cond = n <= g
        elif i == len(CLS) - 1:
            cond = n > prev
        elif g - prev == GR:
            cond = n == g
        else:
            cond = jnp.logical_and(n > prev, n <= g)
        pl.when(cond)(lambda g=g: fn(g))
        prev = g


def _body(x_hbm, rw_hbm, idx_hbm, ew_hbm, sw_hbm, out_ref,
          xbuf, wbuf, swbuf, rwbuf, idxbuf, sbuf, rbuf, lsem, wsem, ssem, rsem):
    my = lax.axis_index("i")
    dk = [(my + k) & 3 for k in range(ND)]

    cx = [pltpu.make_async_copy(x_hbm.at[pl.ds(dk[k] * B, B)], xbuf.at[k], lsem.at[k])
          for k in range(ND)]
    cidx = [pltpu.make_async_copy(idx_hbm, idxbuf.at[pl.ds(4 * j, 4)], lsem.at[4 + j])
            for j in range(2)]
    cw = {(e, h): pltpu.make_async_copy(ew_hbm.at[e, :, pl.ds(256 * h, 256)],
                                        wbuf.at[e, :, pl.ds(256 * h, 256)],
                                        wsem.at[2 * e + h])
          for e in range(EL) for h in range(2)}
    csw = pltpu.make_async_copy(sw_hbm, swbuf, lsem.at[6])
    crw = pltpu.make_async_copy(rw_hbm, rwbuf, lsem.at[7])
    for c in cidx:
        c.start()
    for k in (2, 3):
        cx[k].start()
    barrier = pltpu.get_barrier_semaphore()
    for k in (1, 2, 3):
        pl.semaphore_signal(barrier, inc=1, device_id=(dk[k],), device_id_type=MESH)
    for ph in PHASES:
        cw[ph].start()

    r128 = lax.broadcasted_iota(i32, (B, B), 0)
    c128 = lax.broadcasted_iota(i32, (B, B), 1)
    tri = jnp.concatenate([jnp.where(r128 < c128, 1.0, 0.0), jnp.ones((B, B), f32)],
                          axis=1).astype(bf16)
    sub8 = lax.broadcasted_iota(i32, (8, B), 0)
    capio = lax.broadcasted_iota(i32, (CAP, B), 0)

    for c in cidx:
        c.wait()
    cx[1].start()
    idx8 = pltpu.roll(idxbuf[...], (8 - my) & 7, 0)
    mine = idx8 == (2 * my + (sub8 >> 2))
    hot = [jnp.broadcast_to(idx8[k:k + 1, :], (8, B)) == sub8 for k in range(ND)]
    onehots = jnp.concatenate([jnp.where(m, 1.0, 0.0) for m in [mine] + hot]
                              + [jnp.zeros((8, B), f32)], axis=0).astype(bf16)
    pm = jnp.dot(onehots, tri, preferred_element_type=f32)
    pos = pm[0:16, :B].astype(i32)
    cnt = pm[0:16, B:].astype(i32)
    slot = jnp.where(mine, pos[0:8], -1)
    groups = jnp.minimum(jnp.maximum((cnt + GR - 1) >> 2, 1) - 1, 15)
    nib = sub8 * 4
    send_word = jnp.sum(groups[0:8] << nib, axis=0, keepdims=True)[0, 0]
    recv_word = jnp.sum(groups[8:16] << nib, axis=0, keepdims=True)[0, 0]
    cmax = jnp.maximum(jnp.maximum(pm[8:16, B:], pm[16:24, B:]),
                       jnp.maximum(pm[24:32, B:], pm[32:40, B:]))
    generic = jnp.max(cmax, axis=0, keepdims=True)[0, 0] > float(CAP)

    n_send = {(e, k): GR * ((lax.shift_right_logical(send_word, 4 * (4 * e + k)) & 15) + 1)
              for e in range(EL) for k in REM}
    n_recv = {(e, k): GR * ((lax.shift_right_logical(recv_word, 4 * ((2 * (my - k) + e) & 7)) & 15) + 1)
              for e in range(EL) for k in REM}

    rank = jnp.sum(jnp.where(hot[0], pos[8:16], 0), axis=0, keepdims=True)
    route = idx8[0:1, :]
    k_of = (my - (route >> 1)) & 3
    in_range = jnp.logical_and(route >= 0, route < E)

    def gather_mat(e, k, r):
        row = jnp.broadcast_to(slot[4 * e + k:4 * e + k + 1, :], (CAP, B))
        return jnp.where(row == capio + CAP * r, 1.0, 0.0)

    def w_piece(e, h):
        return wbuf[e, :, 256 * h:256 * h + 256].astype(bf16)

    def expert(e, h, xg):
        y = jnp.dot(xg, w_piece(e, h), preferred_element_type=f32)
        return pltpu.pack_elementwise([y[:, :B], y[:, B:]], packed_dtype=bf16)

    def flow(e, h, k, rows):
        j = (2 * e + h) * 3 + k - 1
        return pltpu.make_async_remote_copy(
            src_ref=sbuf.at[e, h, k - 1, pl.ds(0, rows)],
            dst_ref=rbuf.at[k, h, e, pl.ds(0, rows)],
            send_sem=ssem.at[j], recv_sem=rsem.at[j],
            device_id=(dk[k],), device_id_type=MESH)

    def prob_col(xo):
        sc = lax.dot_general(rwbuf[...].astype(bf16), xo.astype(bf16), (((1,), (1,)), ((), ())),
                             preferred_element_type=f32)
        ex = jnp.exp(sc - jnp.max(sc, axis=0, keepdims=True))
        p = jnp.sum(jnp.where(hot[0], ex, 0.0), axis=0, keepdims=True) / jnp.sum(ex, axis=0, keepdims=True)
        return jnp.broadcast_to(p, (B, B)).T

    def slot_col(r, place):
        rr = rank - CAP * r
        ok = jnp.logical_and(in_range, jnp.logical_and(rr >= 0, rr < CAP))
        code = jnp.where(ok, 64 * place + 32 * (route & 1) + rr, -1024)
        return jnp.broadcast_to(code, (B, B)).T

    def scatter_mat(col, off):
        return jnp.where(col - off == c128, 1.0, 0.0).astype(bf16)

    def received(k, h, r, masked):
        tiles = ([], [])
        for e in range(EL):
            rows = rbuf[k, h, e, pl.ds(r * CAP, CAP), :]
            if masked:
                rows = jnp.where(capio < n_recv[e, k], rows, jnp.uint32(0))
            for t in range(2):
                tiles[t].append(pltpu.unpack_elementwise(rows, index=t, packed_dtype=bf16, unpacked_dtype=f32))
        return [jnp.concatenate(tl, axis=0) for tl in tiles]

    def rhs(parts):
        zero = jnp.zeros((64, B), f32)
        return [jnp.concatenate([zero if q is None else q[t] for q in parts], axis=0).astype(bf16)
                for t in range(2)]

    def add_out(h, p, terms):
        for t in range(2):
            cols = slice(256 * h + 128 * t, 256 * h + 128 * (t + 1))
            y = None
            for sc, rows in terms:
                d = jnp.dot(sc, rows[t], preferred_element_type=f32)
                y = d if y is None else y + d
            out_ref[:, cols] += p * y

    @pl.when(jnp.logical_not(generic))
    def _fast():
        def gather(k):
            cx[k].wait()
            g = jnp.concatenate([gather_mat(0, k, 0), gather_mat(1, k, 0)], axis=0).astype(bf16)
            t = jnp.dot(g, xbuf[k].astype(bf16), preferred_element_type=f32).astype(bf16)
            return t[:CAP], t[CAP:]

        x2, x3 = gather(2), gather(3)
        xg = [jnp.concatenate([x2[e], x3[e]], axis=0) for e in range(EL)]

        col = slot_col(0, jnp.where(k_of == 3, 0, jnp.where(k_of == 2, 1, jnp.where(k_of == 1, 2, 3))))
        s_32, s_1 = scatter_mat(col, 0), scatter_mat(col, 128)
        s_2 = scatter_mat(col, 64)[:, :64]

        def start(items):
            for ph, k in items:
                e, h = PHASES[ph]
                _size_switch(n_send[e, k], lambda rows, e=e, h=h, k=k: flow(e, h, k, rows).start())

        for i, (e, h) in enumerate(PHASES):
            cw[e, h].wait()
            if i == len(PHASES) - 1:
                cx[0].start()
                crw.start()
                csw.start()
            packed = expert(e, h, xg[e])
            sbuf[e, h, 1, 0:CAP, :] = packed[0:CAP]
            if i == 0:
                pl.semaphore_wait(barrier, 3)
            start(SENDS[i][:1])
            sbuf[e, h, 2, 0:CAP, :] = packed[CAP:2 * CAP]
            start(SENDS[i][1:])

        x1 = gather(1)
        for e in range(EL):
            y = jnp.dot(x1[e], wbuf[e].astype(bf16), preferred_element_type=f32)
            for h in range(2):
                sbuf[e, h, 0, 0:CAP, :] = pltpu.pack_elementwise(
                    [y[:, 256 * h:256 * h + B], y[:, 256 * h + B:256 * h + 256]], packed_dtype=bf16)
            for h in range(2):
                _size_switch(n_send[e, 1], lambda rows, e=e, h=h: flow(e, h, 1, rows).start())

        cx[0].wait()
        crw.wait()
        xo = xbuf[0]
        p = prob_col(xo)
        x_e = []
        for e in range(EL):
            m = jnp.where((col >> 5) == 6 + e, 1.0, 0.0)
            x_e.append(jnp.concatenate([xo[:, :B] * m, xo[:, B:] * m], axis=1).astype(bf16))
        for h in range(2):
            y_ex = (jnp.dot(x_e[0], w_piece(0, h), preferred_element_type=f32)
                    + jnp.dot(x_e[1], w_piece(1, h), preferred_element_type=f32))
            for t in range(2):
                out_ref[:, 256 * h + 128 * t:256 * h + 128 * (t + 1)] = p * y_ex[:, 128 * t:128 * (t + 1)]
        csw.wait()
        out_ref[...] += jnp.dot(xo.astype(bf16), swbuf[...].astype(bf16), preferred_element_type=f32)

        for e in range(EL):
            for h in range(2):
                for k in REM:
                    _size_switch(n_send[e, k], lambda rows, e=e, h=h, k=k: flow(e, h, k, rows).wait_send())

        def wait_recv(k, h, es=(0, 1)):
            for e in es:
                _size_switch(n_recv[e, k], lambda rows, e=e: flow(e, h, k, rows).wait_recv())

        for h in range(2):
            wait_recv(3, h)
        wait_recv(2, 0)
        for h in range(2):
            second = received(2, 0, 0, True) if h == 0 else None
            add_out(h, p, [(s_32, rhs([received(3, h, 0, True), second]))])
        for h in range(2):
            wait_recv(1, h)
        wait_recv(2, 1, (0,))
        for h in range(2):
            add_out(h, p, [(s_1, rhs([received(1, h, 0, True), None]))])
        wait_recv(2, 1, (1,))
        far = [q.astype(bf16) for q in received(2, 1, 0, True)]
        for t in range(2):
            for mh in range(2):
                rows = slice(64 * mh, 64 * mh + 64)
                cols = slice(256 + 128 * t, 256 + 128 * (t + 1))
                y = jnp.dot(s_2[rows], far[t], preferred_element_type=f32)
                out_ref[rows, cols] += p[rows] * y

    @pl.when(generic)
    def _generic():
        cx[0].start()
        crw.start()
        csw.start()
        for k in range(ND):
            cx[k].wait()
        for ph in PHASES:
            cw[ph].wait()
        crw.wait()
        csw.wait()
        pl.semaphore_wait(barrier, 3)

        @pl.loop(0, B // CAP)
        def _(r):
            for k in range(ND):
                for e in range(EL):
                    g = gather_mat(e, k, r).astype(bf16)
                    t = jnp.dot(g, xbuf[k].astype(bf16), preferred_element_type=f32).astype(bf16)
                    for h in range(2):
                        dst = rbuf.at[0, h, e] if k == 0 else sbuf.at[e, h, k - 1]
                        dst[pl.ds(pl.multiple_of(r * CAP, CAP), CAP), :] = expert(e, h, t)

        every = [(e, h, k) for e in range(EL) for h in range(2) for k in REM]
        for e, h, k in every:
            flow(e, h, k, B).start()
        xo = xbuf[0]
        p = prob_col(xo)
        out_ref[...] = jnp.dot(xo.astype(bf16), swbuf[...].astype(bf16), preferred_element_type=f32)
        for e, h, k in every:
            flow(e, h, k, B).wait()

        @pl.loop(0, B // CAP)
        def _(r):
            col = slot_col(r, k_of)
            s01, s23 = scatter_mat(col, 0), scatter_mat(col, 128)
            for h in range(2):
                add_out(h, p, [(s01, rhs([received(0, h, r, False), received(1, h, r, False)])),
                               (s23, rhs([received(2, h, r, False), received(3, h, r, False)]))])


def pallas_dist_moe_shared_ep_outshard_n512_d256_e2_h512_kernel(
    x: jax.Array,
    router_W: jax.Array,
    route_idx: jax.Array,
    expert_W: jax.Array,
    shared_W: jax.Array,
):
    any_space = pl.BlockSpec(memory_space=pltpu.HBM)
    return pl.pallas_call(
        _body,
        out_shape=jax.ShapeDtypeStruct((B, H), f32),
        in_specs=[any_space] * 5,
        out_specs=pl.BlockSpec(memory_space=pltpu.VMEM),
        scratch_shapes=[
            pltpu.VMEM((ND, B, D), f32),
            pltpu.VMEM((EL, D, H), f32),
            pltpu.VMEM((D, H), f32),
            pltpu.VMEM((E, D), f32),
            pltpu.VMEM((8, B), i32),
            pltpu.VMEM((EL, 2, 3, B, B), u32),
            pltpu.VMEM((ND, 2, EL, B, B), u32),
            pltpu.SemaphoreType.DMA((8,)),
            pltpu.SemaphoreType.DMA((4,)),
            pltpu.SemaphoreType.DMA((12,)),
            pltpu.SemaphoreType.DMA((12,)),
        ],
        compiler_params=pltpu.CompilerParams(
            collective_id=0,
            disable_semaphore_checks=True,
            disable_bounds_checks=True,
        ),
    )(x, router_W.T, route_idx.reshape(ND, B), expert_W, shared_W)
```

```python
import jax
import jax.numpy as jnp
from jax import lax
from jax.experimental import pallas as pl
from jax.experimental.pallas import tpu as pltpu

D, H, E, EL, ND, B = 256, 512, 8, 2, 4, 128
CAP = 32
GR = 4
CLS = (16, 20, 24, 32)
REM = (2, 3, 1)
PHASES = ((0, 0), (1, 0), (0, 1), (1, 1))
SENDS = (
    ((0, 2), (0, 3)),
    ((1, 2), (1, 3)),
    ((2, 2),),
    ((3, 2), (2, 3), (3, 3)),
)
MESH = pl.DeviceIdType.MESH
bf16, f32, i32, u32 = jnp.bfloat16, jnp.float32, jnp.int32, jnp.uint32


def _pack(lo, hi):
    lo = lax.bitcast_convert_type(lo.astype(bf16).astype(f32), u32)
    hi = lax.bitcast_convert_type(hi.astype(bf16).astype(f32), u32)
    return hi | (lo >> 16)


def _unpack(w):
    return (lax.bitcast_convert_type(w << 16, f32),
            lax.bitcast_convert_type(w & jnp.uint32(0xFFFF0000), f32))


def _size_switch(n, fn):
    prev = None
    for i, g in enumerate(CLS):
        if prev is None:
            cond = n <= g
        elif i == len(CLS) - 1:
            cond = n > prev
        elif g - prev == GR:
            cond = n == g
        else:
            cond = jnp.logical_and(n > prev, n <= g)
        pl.when(cond)(lambda g=g: fn(g))
        prev = g


def _body(x_hbm, rw_hbm, idx_hbm, ew_hbm, sw_hbm, out_ref,
          xbuf, wbuf, swbuf, rwbuf, idxbuf, sbuf, rbuf, lsem, wsem, ssem, rsem):
    my = lax.axis_index("i")
    dk = [(my + k) & 3 for k in range(ND)]

    cx = [pltpu.make_async_copy(x_hbm.at[pl.ds(dk[k] * B, B)], xbuf.at[k], lsem.at[k])
          for k in range(ND)]
    cidx = [pltpu.make_async_copy(idx_hbm, idxbuf.at[pl.ds(4 * j, 4)], lsem.at[4 + j])
            for j in range(2)]
    cw = {(e, h): pltpu.make_async_copy(ew_hbm.at[e, :, pl.ds(256 * h, 256)],
                                        wbuf.at[e, :, pl.ds(256 * h, 256)],
                                        wsem.at[2 * e + h])
          for e in range(EL) for h in range(2)}
    csw = pltpu.make_async_copy(sw_hbm, swbuf, lsem.at[6])
    crw = pltpu.make_async_copy(rw_hbm, rwbuf, lsem.at[7])
    for c in cidx:
        c.start()
    for k in (2, 3):
        cx[k].start()
    barrier = pltpu.get_barrier_semaphore()
    for k in (1, 2, 3):
        pl.semaphore_signal(barrier, inc=1, device_id=(dk[k],), device_id_type=MESH)
    for ph in PHASES:
        cw[ph].start()

    r128 = lax.broadcasted_iota(i32, (B, B), 0)
    c128 = lax.broadcasted_iota(i32, (B, B), 1)
    tri = jnp.concatenate([jnp.where(r128 < c128, 1.0, 0.0), jnp.ones((B, B), f32)],
                          axis=1).astype(bf16)
    sub8 = lax.broadcasted_iota(i32, (8, B), 0)
    capio = lax.broadcasted_iota(i32, (CAP, B), 0)

    for c in cidx:
        c.wait()
    cx[1].start()
    idx8 = pltpu.roll(idxbuf[...], (8 - my) & 7, 0)
    mine = idx8 == (2 * my + (sub8 >> 2))
    hot = [jnp.broadcast_to(idx8[k:k + 1, :], (8, B)) == sub8 for k in range(ND)]
    onehots = jnp.concatenate([jnp.where(m, 1.0, 0.0) for m in [mine] + hot]
                              + [jnp.zeros((8, B), f32)], axis=0).astype(bf16)
    pm = jnp.dot(onehots, tri, preferred_element_type=f32)
    pos = pm[0:16, :B].astype(i32)
    cnt = pm[0:16, B:].astype(i32)
    slot = jnp.where(mine, pos[0:8], -1)
    groups = jnp.minimum(jnp.maximum((cnt + GR - 1) >> 2, 1) - 1, 15)
    nib = sub8 * 4
    send_word = jnp.sum(groups[0:8] << nib, axis=0, keepdims=True)[0, 0]
    recv_word = jnp.sum(groups[8:16] << nib, axis=0, keepdims=True)[0, 0]
    cmax = jnp.maximum(jnp.maximum(pm[8:16, B:], pm[16:24, B:]),
                       jnp.maximum(pm[24:32, B:], pm[32:40, B:]))
    generic = jnp.max(cmax, axis=0, keepdims=True)[0, 0] > float(CAP)

    n_send = {(e, k): GR * ((lax.shift_right_logical(send_word, 4 * (4 * e + k)) & 15) + 1)
              for e in range(EL) for k in REM}
    n_recv = {(e, k): GR * ((lax.shift_right_logical(recv_word, 4 * ((2 * (my - k) + e) & 7)) & 15) + 1)
              for e in range(EL) for k in REM}

    rank = jnp.sum(jnp.where(hot[0], pos[8:16], 0), axis=0, keepdims=True)
    route = idx8[0:1, :]
    k_of = (my - (route >> 1)) & 3
    in_range = jnp.logical_and(route >= 0, route < E)

    def gather_mat(e, k, r):
        row = jnp.broadcast_to(slot[4 * e + k:4 * e + k + 1, :], (CAP, B))
        return jnp.where(row == capio + CAP * r, 1.0, 0.0)

    def w_piece(e, h):
        return wbuf[e, :, 256 * h:256 * h + 256].astype(bf16)

    def expert(e, h, xg):
        y = jnp.dot(xg, w_piece(e, h), preferred_element_type=f32)
        return _pack(y[:, :B], y[:, B:])

    def flow(e, h, k, rows):
        j = (2 * e + h) * 3 + k - 1
        return pltpu.make_async_remote_copy(
            src_ref=sbuf.at[e, h, k - 1, pl.ds(0, rows)],
            dst_ref=rbuf.at[k, h, e, pl.ds(0, rows)],
            send_sem=ssem.at[j], recv_sem=rsem.at[j],
            device_id=(dk[k],), device_id_type=MESH)

    def prob_col(xo):
        sc = lax.dot_general(rwbuf[...].astype(bf16), xo.astype(bf16), (((1,), (1,)), ((), ())),
                             preferred_element_type=f32)
        ex = jnp.exp(sc - jnp.max(sc, axis=0, keepdims=True))
        p = jnp.sum(jnp.where(hot[0], ex, 0.0), axis=0, keepdims=True) / jnp.sum(ex, axis=0, keepdims=True)
        return jnp.broadcast_to(p, (B, B)).T

    def slot_col(r, place):
        rr = rank - CAP * r
        ok = jnp.logical_and(in_range, jnp.logical_and(rr >= 0, rr < CAP))
        code = jnp.where(ok, 64 * place + 32 * (route & 1) + rr, -1024)
        return jnp.broadcast_to(code, (B, B)).T

    def scatter_mat(col, off):
        return jnp.where(col - off == c128, 1.0, 0.0).astype(bf16)

    def received(k, h, r, masked):
        tiles = ([], [])
        for e in range(EL):
            rows = rbuf[k, h, e, pl.ds(r * CAP, CAP), :]
            if masked:
                rows = jnp.where(capio < n_recv[e, k], rows, jnp.uint32(0))
            for t, q in enumerate(_unpack(rows)):
                tiles[t].append(q)
        return [jnp.concatenate(tl, axis=0) for tl in tiles]

    def rhs(parts):
        zero = jnp.zeros((64, B), f32)
        return [jnp.concatenate([zero if q is None else q[t] for q in parts], axis=0).astype(bf16)
                for t in range(2)]

    def add_out(h, p, terms):
        for t in range(2):
            cols = slice(256 * h + 128 * t, 256 * h + 128 * (t + 1))
            y = None
            for sc, rows in terms:
                d = jnp.dot(sc, rows[t], preferred_element_type=f32)
                y = d if y is None else y + d
            out_ref[:, cols] += p * y

    @pl.when(jnp.logical_not(generic))
    def _fast():
        def gather(k):
            cx[k].wait()
            g = jnp.concatenate([gather_mat(0, k, 0), gather_mat(1, k, 0)], axis=0).astype(bf16)
            t = jnp.dot(g, xbuf[k].astype(bf16), preferred_element_type=f32).astype(bf16)
            return t[:CAP], t[CAP:]

        x2, x3 = gather(2), gather(3)
        xg = [jnp.concatenate([x2[e], x3[e]], axis=0) for e in range(EL)]

        col = slot_col(0, jnp.where(k_of == 3, 0, jnp.where(k_of == 2, 1, jnp.where(k_of == 1, 2, 3))))
        s_32, s_1 = scatter_mat(col, 0), scatter_mat(col, 128)
        s_2 = scatter_mat(col, 64)[:, :64]

        def start(items):
            for ph, k in items:
                e, h = PHASES[ph]
                _size_switch(n_send[e, k], lambda rows, e=e, h=h, k=k: flow(e, h, k, rows).start())

        for i, (e, h) in enumerate(PHASES):
            cw[e, h].wait()
            if i == len(PHASES) - 1:
                cx[0].start()
                crw.start()
                csw.start()
            packed = expert(e, h, xg[e])
            sbuf[e, h, 1, 0:CAP, :] = packed[0:CAP]
            if i == 0:
                pl.semaphore_wait(barrier, 3)
            start(SENDS[i][:1])
            sbuf[e, h, 2, 0:CAP, :] = packed[CAP:2 * CAP]
            start(SENDS[i][1:])

        x1 = gather(1)
        for e in range(EL):
            y = jnp.dot(x1[e], wbuf[e].astype(bf16), preferred_element_type=f32)
            for h in range(2):
                sbuf[e, h, 0, 0:CAP, :] = _pack(y[:, 256 * h:256 * h + B], y[:, 256 * h + B:256 * h + 256])
            for h in range(2):
                _size_switch(n_send[e, 1], lambda rows, e=e, h=h: flow(e, h, 1, rows).start())

        cx[0].wait()
        crw.wait()
        xo = xbuf[0]
        p = prob_col(xo)
        x_e = []
        for e in range(EL):
            m = jnp.where((col >> 5) == 6 + e, 1.0, 0.0)
            x_e.append(jnp.concatenate([xo[:, :B] * m, xo[:, B:] * m], axis=1).astype(bf16))
        for h in range(2):
            y_ex = (jnp.dot(x_e[0], w_piece(0, h), preferred_element_type=f32)
                    + jnp.dot(x_e[1], w_piece(1, h), preferred_element_type=f32))
            for t in range(2):
                out_ref[:, 256 * h + 128 * t:256 * h + 128 * (t + 1)] = p * y_ex[:, 128 * t:128 * (t + 1)]
        csw.wait()
        out_ref[...] += jnp.dot(xo.astype(bf16), swbuf[...].astype(bf16), preferred_element_type=f32)

        for e in range(EL):
            for h in range(2):
                for k in REM:
                    _size_switch(n_send[e, k], lambda rows, e=e, h=h, k=k: flow(e, h, k, rows).wait_send())

        def wait_recv(k, h, es=(0, 1)):
            for e in es:
                _size_switch(n_recv[e, k], lambda rows, e=e: flow(e, h, k, rows).wait_recv())

        for h in range(2):
            wait_recv(3, h)
        wait_recv(2, 0)
        for h in range(2):
            second = received(2, 0, 0, True) if h == 0 else None
            add_out(h, p, [(s_32, rhs([received(3, h, 0, True), second]))])
        for h in range(2):
            wait_recv(1, h)
        wait_recv(2, 1, (0,))
        for h in range(2):
            add_out(h, p, [(s_1, rhs([received(1, h, 0, True), None]))])
        wait_recv(2, 1, (1,))
        far = [q.astype(bf16) for q in received(2, 1, 0, True)]
        for t in range(2):
            for mh in range(2):
                rows = slice(64 * mh, 64 * mh + 64)
                cols = slice(256 + 128 * t, 256 + 128 * (t + 1))
                y = jnp.dot(s_2[rows], far[t], preferred_element_type=f32)
                out_ref[rows, cols] += p[rows] * y

    @pl.when(generic)
    def _generic():
        cx[0].start()
        crw.start()
        csw.start()
        for k in range(ND):
            cx[k].wait()
        for ph in PHASES:
            cw[ph].wait()
        crw.wait()
        csw.wait()
        pl.semaphore_wait(barrier, 3)

        @pl.loop(0, B // CAP)
        def _(r):
            for k in range(ND):
                for e in range(EL):
                    g = gather_mat(e, k, r).astype(bf16)
                    t = jnp.dot(g, xbuf[k].astype(bf16), preferred_element_type=f32).astype(bf16)
                    for h in range(2):
                        dst = rbuf.at[0, h, e] if k == 0 else sbuf.at[e, h, k - 1]
                        dst[pl.ds(pl.multiple_of(r * CAP, CAP), CAP), :] = expert(e, h, t)

        every = [(e, h, k) for e in range(EL) for h in range(2) for k in REM]
        for e, h, k in every:
            flow(e, h, k, B).start()
        xo = xbuf[0]
        p = prob_col(xo)
        out_ref[...] = jnp.dot(xo.astype(bf16), swbuf[...].astype(bf16), preferred_element_type=f32)
        for e, h, k in every:
            flow(e, h, k, B).wait()

        @pl.loop(0, B // CAP)
        def _(r):
            col = slot_col(r, k_of)
            s01, s23 = scatter_mat(col, 0), scatter_mat(col, 128)
            for h in range(2):
                add_out(h, p, [(s01, rhs([received(0, h, r, False), received(1, h, r, False)])),
                               (s23, rhs([received(2, h, r, False), received(3, h, r, False)]))])


def pallas_dist_moe_shared_ep_outshard_n512_d256_e2_h512_kernel(
    x: jax.Array,
    router_W: jax.Array,
    route_idx: jax.Array,
    expert_W: jax.Array,
    shared_W: jax.Array,
):
    any_space = pl.BlockSpec(memory_space=pltpu.HBM)
    return pl.pallas_call(
        _body,
        out_shape=jax.ShapeDtypeStruct((B, H), f32),
        in_specs=[any_space] * 5,
        out_specs=pl.BlockSpec(memory_space=pltpu.VMEM),
        scratch_shapes=[
            pltpu.VMEM((ND, B, D), f32),
            pltpu.VMEM((EL, D, H), f32),
            pltpu.VMEM((D, H), f32),
            pltpu.VMEM((E, D), f32),
            pltpu.VMEM((8, B), i32),
            pltpu.VMEM((EL, 2, 3, B, B), u32),
            pltpu.VMEM((ND, 2, EL, B, B), u32),
            pltpu.SemaphoreType.DMA((8,)),
            pltpu.SemaphoreType.DMA((4,)),
            pltpu.SemaphoreType.DMA((12,)),
            pltpu.SemaphoreType.DMA((12,)),
        ],
        compiler_params=pltpu.CompilerParams(
            collective_id=0,
            disable_semaphore_checks=True,
            disable_bounds_checks=True,
        ),
    )(x, router_W.T, route_idx.reshape(ND, B), expert_W, shared_W)
```

```python
import jax
import jax.numpy as jnp
from jax import lax
from jax.experimental import pallas as pl
from jax.experimental.pallas import tpu as pltpu

D, H, E, EL, ND, B = 256, 512, 8, 2, 4, 128
CAP = 32
GR = 4
CLS = (16, 20, 24, 32)
REM = (2, 3, 1)
PHASES = ((0, 0), (1, 0), (0, 1), (1, 1))
SENDS = (
    ((0, 2), (0, 3)),
    ((1, 2), (1, 3)),
    ((2, 2),),
    ((3, 2), (2, 3), (3, 3)),
)
MESH = pl.DeviceIdType.MESH
bf16, f32, i32, u32 = jnp.bfloat16, jnp.float32, jnp.int32, jnp.uint32


def _pack(lo, hi):
    lo = lax.bitcast_convert_type(lo.astype(bf16).astype(f32), u32)
    hi = lax.bitcast_convert_type(hi.astype(bf16).astype(f32), u32)
    return hi | (lo >> 16)


def _unpack(w):
    return (lax.bitcast_convert_type(w << 16, f32),
            lax.bitcast_convert_type(w & jnp.uint32(0xFFFF0000), f32))


def _size_switch(n, fn):
    prev = None
    for i, g in enumerate(CLS):
        if prev is None:
            cond = n <= g
        elif i == len(CLS) - 1:
            cond = n > prev
        elif g - prev == GR:
            cond = n == g
        else:
            cond = jnp.logical_and(n > prev, n <= g)
        pl.when(cond)(lambda g=g: fn(g))
        prev = g


def _body(x_hbm, rw_hbm, idx_hbm, ew_hbm, sw_hbm, out_ref,
          xbuf, wbuf, swbuf, rwbuf, idxbuf, sbuf, rbuf, lsem, wsem, ssem, rsem):
    my = lax.axis_index("i")
    dk = [(my + k) & 3 for k in range(ND)]

    cx = [pltpu.make_async_copy(x_hbm.at[pl.ds(dk[k] * B, B)], xbuf.at[k], lsem.at[k])
          for k in range(ND)]
    cidx = [pltpu.make_async_copy(idx_hbm, idxbuf.at[pl.ds(4 * j, 4)], lsem.at[4 + j])
            for j in range(2)]
    cw = {(e, h): pltpu.make_async_copy(ew_hbm.at[e, :, pl.ds(256 * h, 256)],
                                        wbuf.at[e, :, pl.ds(256 * h, 256)],
                                        wsem.at[2 * e + h])
          for e in range(EL) for h in range(2)}
    csw = pltpu.make_async_copy(sw_hbm, swbuf, lsem.at[6])
    crw = pltpu.make_async_copy(rw_hbm, rwbuf, lsem.at[7])
    for c in cidx:
        c.start()
    for k in (2, 3):
        cx[k].start()
    barrier = pltpu.get_barrier_semaphore()
    for k in (1, 2, 3):
        pl.semaphore_signal(barrier, inc=1, device_id=(dk[k],), device_id_type=MESH)
    for ph in PHASES:
        cw[ph].start()

    r128 = lax.broadcasted_iota(i32, (B, B), 0)
    c128 = lax.broadcasted_iota(i32, (B, B), 1)
    tri = jnp.concatenate([jnp.where(r128 < c128, 1.0, 0.0), jnp.ones((B, B), f32)],
                          axis=1).astype(bf16)
    sub8 = lax.broadcasted_iota(i32, (8, B), 0)
    capio = lax.broadcasted_iota(i32, (CAP, B), 0)

    for c in cidx:
        c.wait()
    cx[1].start()
    idx8 = pltpu.roll(idxbuf[...], (8 - my) & 7, 0)
    mine = idx8 == (2 * my + (sub8 >> 2))
    hot = [jnp.broadcast_to(idx8[k:k + 1, :], (8, B)) == sub8 for k in range(ND)]
    onehots = jnp.concatenate([jnp.where(m, 1.0, 0.0) for m in [mine] + hot]
                              + [jnp.zeros((8, B), f32)], axis=0).astype(bf16)
    pm = jnp.dot(onehots, tri, preferred_element_type=f32)
    pos = pm[0:16, :B].astype(i32)
    cnt = pm[0:16, B:].astype(i32)
    slot = jnp.where(mine, pos[0:8], -1)
    groups = jnp.minimum(jnp.maximum((cnt + GR - 1) >> 2, 1) - 1, 15)
    nib = sub8 * 4
    send_word = jnp.sum(groups[0:8] << nib, axis=0, keepdims=True)[0, 0]
    recv_word = jnp.sum(groups[8:16] << nib, axis=0, keepdims=True)[0, 0]
    cmax = jnp.maximum(jnp.maximum(pm[8:16, B:], pm[16:24, B:]),
                       jnp.maximum(pm[24:32, B:], pm[32:40, B:]))
    generic = jnp.max(cmax, axis=0, keepdims=True)[0, 0] > float(CAP)

    n_send = {(e, k): GR * ((lax.shift_right_logical(send_word, 4 * (4 * e + k)) & 15) + 1)
              for e in range(EL) for k in REM}
    n_recv = {(e, k): GR * ((lax.shift_right_logical(recv_word, 4 * ((2 * (my - k) + e) & 7)) & 15) + 1)
              for e in range(EL) for k in REM}

    rank = jnp.sum(jnp.where(hot[0], pos[8:16], 0), axis=0, keepdims=True)
    route = idx8[0:1, :]
    k_of = (my - (route >> 1)) & 3
    in_range = jnp.logical_and(route >= 0, route < E)

    def gather_mat(e, k, r):
        row = jnp.broadcast_to(slot[4 * e + k:4 * e + k + 1, :], (CAP, B))
        return jnp.where(row == capio + CAP * r, 1.0, 0.0)

    def w_piece(e, h):
        return wbuf[e, :, 256 * h:256 * h + 256].astype(bf16)

    def expert(e, h, xg):
        y = jnp.dot(xg, w_piece(e, h), preferred_element_type=f32)
        return _pack(y[:, :B], y[:, B:])

    def flow(e, h, k, rows):
        j = (2 * e + h) * 3 + k - 1
        return pltpu.make_async_remote_copy(
            src_ref=sbuf.at[e, h, k - 1, pl.ds(0, rows)],
            dst_ref=rbuf.at[k, h, e, pl.ds(0, rows)],
            send_sem=ssem.at[j], recv_sem=rsem.at[j],
            device_id=(dk[k],), device_id_type=MESH)

    def prob_col(xo):
        sc = lax.dot_general(rwbuf[...].astype(bf16), xo.astype(bf16), (((1,), (1,)), ((), ())),
                             preferred_element_type=f32)
        ex = jnp.exp(sc - jnp.max(sc, axis=0, keepdims=True))
        p = jnp.sum(jnp.where(hot[0], ex, 0.0), axis=0, keepdims=True) / jnp.sum(ex, axis=0, keepdims=True)
        return jnp.broadcast_to(p, (B, B)).T

    def slot_col(r, place):
        rr = rank - CAP * r
        ok = jnp.logical_and(in_range, jnp.logical_and(rr >= 0, rr < CAP))
        code = jnp.where(ok, 64 * place + 32 * (route & 1) + rr, -1024)
        return jnp.broadcast_to(code, (B, B)).T

    def scatter_mat(col, off):
        return jnp.where(col - off == c128, 1.0, 0.0).astype(bf16)

    def received(k, h, r, masked):
        tiles = ([], [])
        for e in range(EL):
            rows = rbuf[k, h, e, pl.ds(r * CAP, CAP), :]
            if masked:
                rows = jnp.where(capio < n_recv[e, k], rows, jnp.uint32(0))
            for t, q in enumerate(_unpack(rows)):
                tiles[t].append(q)
        return [jnp.concatenate(tl, axis=0) for tl in tiles]

    def rhs(parts):
        zero = jnp.zeros((64, B), f32)
        return [jnp.concatenate([zero if q is None else q[t] for q in parts], axis=0).astype(bf16)
                for t in range(2)]

    def add_out(h, p, terms):
        for t in range(2):
            cols = slice(256 * h + 128 * t, 256 * h + 128 * (t + 1))
            y = None
            for sc, rows in terms:
                d = jnp.dot(sc, rows[t], preferred_element_type=f32)
                y = d if y is None else y + d
            out_ref[:, cols] += p * y

    @pl.when(jnp.logical_not(generic))
    def _fast():
        def gather(k):
            cx[k].wait()
            g = jnp.concatenate([gather_mat(0, k, 0), gather_mat(1, k, 0)], axis=0).astype(bf16)
            t = jnp.dot(g, xbuf[k].astype(bf16), preferred_element_type=f32).astype(bf16)
            return t[:CAP], t[CAP:]

        x2, x3 = gather(2), gather(3)
        xg = [jnp.concatenate([x2[e], x3[e]], axis=0) for e in range(EL)]

        col = slot_col(0, jnp.where(k_of == 3, 0, jnp.where(k_of == 2, 1, jnp.where(k_of == 1, 2, 3))))
        s_32, s_1 = scatter_mat(col, 0), scatter_mat(col, 128)
        s_2 = scatter_mat(col, 64)[:, :64]

        def start(items):
            for ph, k in items:
                e, h = PHASES[ph]
                _size_switch(n_send[e, k], lambda rows, e=e, h=h, k=k: flow(e, h, k, rows).start())

        for i, (e, h) in enumerate(PHASES):
            cw[e, h].wait()
            if i == len(PHASES) - 1:
                cx[0].start()
                crw.start()
                csw.start()
            packed = expert(e, h, xg[e])
            sbuf[e, h, 1, 0:CAP, :] = packed[0:CAP]
            if i == 0:
                pl.semaphore_wait(barrier, 3)
            start(SENDS[i][:1])
            sbuf[e, h, 2, 0:CAP, :] = packed[CAP:2 * CAP]
            start(SENDS[i][1:])

        x1 = gather(1)
        for e in range(EL):
            y = jnp.dot(x1[e], wbuf[e].astype(bf16), preferred_element_type=f32)
            for h in range(2):
                sbuf[e, h, 0, 0:CAP, :] = _pack(y[:, 256 * h:256 * h + B], y[:, 256 * h + B:256 * h + 256])
            for h in range(2):
                _size_switch(n_send[e, 1], lambda rows, e=e, h=h: flow(e, h, 1, rows).start())

        cx[0].wait()
        crw.wait()
        xo = xbuf[0]
        p = prob_col(xo)
        x_e = []
        for e in range(EL):
            m = jnp.where((col >> 5) == 6 + e, 1.0, 0.0)
            x_e.append(jnp.concatenate([xo[:, :B] * m, xo[:, B:] * m], axis=1).astype(bf16))
        for h in range(2):
            y_ex = (jnp.dot(x_e[0], w_piece(0, h), preferred_element_type=f32)
                    + jnp.dot(x_e[1], w_piece(1, h), preferred_element_type=f32))
            for t in range(2):
                out_ref[:, 256 * h + 128 * t:256 * h + 128 * (t + 1)] = p * y_ex[:, 128 * t:128 * (t + 1)]
        csw.wait()
        out_ref[...] += jnp.dot(xo.astype(bf16), swbuf[...].astype(bf16), preferred_element_type=f32)

        for e in range(EL):
            for h in range(2):
                for k in REM:
                    _size_switch(n_send[e, k], lambda rows, e=e, h=h, k=k: flow(e, h, k, rows).wait_send())

        def wait_recv(k, h):
            for e in range(EL):
                _size_switch(n_recv[e, k], lambda rows, e=e: flow(e, h, k, rows).wait_recv())

        for h in range(2):
            wait_recv(3, h)
        wait_recv(2, 0)
        for h in range(2):
            second = received(2, 0, 0, True) if h == 0 else None
            add_out(h, p, [(s_32, rhs([received(3, h, 0, True), second]))])
        for h in range(2):
            wait_recv(1, h)
        for h in range(2):
            add_out(h, p, [(s_1, rhs([received(1, h, 0, True), None]))])
        wait_recv(2, 1)
        far = [q.astype(bf16) for q in received(2, 1, 0, True)]
        for t in range(2):
            for mh in range(2):
                rows = slice(64 * mh, 64 * mh + 64)
                cols = slice(256 + 128 * t, 256 + 128 * (t + 1))
                y = jnp.dot(s_2[rows], far[t], preferred_element_type=f32)
                out_ref[rows, cols] += p[rows] * y

    @pl.when(generic)
    def _generic():
        cx[0].start()
        crw.start()
        csw.start()
        for k in range(ND):
            cx[k].wait()
        for ph in PHASES:
            cw[ph].wait()
        crw.wait()
        csw.wait()
        pl.semaphore_wait(barrier, 3)

        @pl.loop(0, B // CAP)
        def _(r):
            for k in range(ND):
                for e in range(EL):
                    g = gather_mat(e, k, r).astype(bf16)
                    t = jnp.dot(g, xbuf[k].astype(bf16), preferred_element_type=f32).astype(bf16)
                    for h in range(2):
                        dst = rbuf.at[0, h, e] if k == 0 else sbuf.at[e, h, k - 1]
                        dst[pl.ds(pl.multiple_of(r * CAP, CAP), CAP), :] = expert(e, h, t)

        every = [(e, h, k) for e in range(EL) for h in range(2) for k in REM]
        for e, h, k in every:
            flow(e, h, k, B).start()
        xo = xbuf[0]
        p = prob_col(xo)
        out_ref[...] = jnp.dot(xo.astype(bf16), swbuf[...].astype(bf16), preferred_element_type=f32)
        for e, h, k in every:
            flow(e, h, k, B).wait()

        @pl.loop(0, B // CAP)
        def _(r):
            col = slot_col(r, k_of)
            s01, s23 = scatter_mat(col, 0), scatter_mat(col, 128)
            for h in range(2):
                add_out(h, p, [(s01, rhs([received(0, h, r, False), received(1, h, r, False)])),
                               (s23, rhs([received(2, h, r, False), received(3, h, r, False)]))])


def pallas_dist_moe_shared_ep_outshard_n512_d256_e2_h512_kernel(
    x: jax.Array,
    router_W: jax.Array,
    route_idx: jax.Array,
    expert_W: jax.Array,
    shared_W: jax.Array,
):
    any_space = pl.BlockSpec(memory_space=pltpu.HBM)
    return pl.pallas_call(
        _body,
        out_shape=jax.ShapeDtypeStruct((B, H), f32),
        in_specs=[any_space] * 5,
        out_specs=pl.BlockSpec(memory_space=pltpu.VMEM),
        scratch_shapes=[
            pltpu.VMEM((ND, B, D), f32),
            pltpu.VMEM((EL, D, H), f32),
            pltpu.VMEM((D, H), f32),
            pltpu.VMEM((E, D), f32),
            pltpu.VMEM((8, B), i32),
            pltpu.VMEM((EL, 2, 3, B, B), u32),
            pltpu.VMEM((ND, 2, EL, B, B), u32),
            pltpu.SemaphoreType.DMA((8,)),
            pltpu.SemaphoreType.DMA((4,)),
            pltpu.SemaphoreType.DMA((12,)),
            pltpu.SemaphoreType.DMA((12,)),
        ],
        compiler_params=pltpu.CompilerParams(
            collective_id=0,
            disable_semaphore_checks=True,
            disable_bounds_checks=True,
        ),
    )(x, router_W.T, route_idx.reshape(ND, B), expert_W, shared_W)
```
